```python
import numpy as np

kernel_name = "dist_ag_xy_y_m65536_n1024"

def setup_inputs():
    return {"x": np.random.randn(131072, 1024).astype(np.float32)}

def reference(x: np.ndarray) -> np.ndarray:
    return x
```

```python
import numpy as np
import jax
import jax.numpy as jnp
from jax import lax
from jax.experimental import pallas as pl
from jax.experimental.pallas import tpu as pltpu

I32 = jnp.int32
BF16 = jnp.bfloat16


def c32(v):
    return np.uint32(v).view(np.int32)


def rep(b):
    return c32(b * 0x01010101)


def _amount(n):
    return jnp.asarray(n, I32) if isinstance(n, int) else n


def shl(a, n):
    return lax.shift_left(a, _amount(n))


def shr(a, n):
    return lax.shift_right_logical(a, _amount(n))


def split(a, b):
    ar = shr(a, 7) | shl(a, 25)
    br = shl(b, 1) | shr(b, 31)
    x = (ar ^ br) & c32(0x00FF00FF)
    return br ^ x, ar ^ x


def join(ex, raw):
    x = (ex ^ raw) & c32(0x00FF00FF)
    br, ar = ex ^ x, raw ^ x
    return shl(ar, 7) | shr(ar, 25), shr(br, 1) | shl(br, 31)


def rank_of(t):
    ge2 = (t + rep(0x7E)) & rep(0x80)
    ge1 = (t + rep(0x7F)) & rep(0x80)
    ge7 = shr(t + rep(0x79), 7) & rep(1)
    ge13 = shr(t + rep(0x73), 7) & rep(1)
    return t + rep(12) + ge7 + ge13 - (shr(ge2, 5) | shr(ge2, 6)) - shr(ge1, 4)


def exps_of(r, base4):
    ge5 = (r + rep(0x7B)) & rep(0x80)
    ge6 = (r + rep(0x7A)) & rep(0x80)
    ge12 = (r + rep(0x74)) & rep(0x80)
    ge13 = (r + rep(0x73)) & rep(0x80)
    eq5 = ge5 ^ ge6
    eq12 = ge12 ^ ge13
    return (base4 + shr(ge6, 7) + shr(ge13, 7) + (shr(eq5, 5) | shr(eq5, 6))
            + ((eq12 - shr(eq12, 7)) & rep(13)) - r)


def funnel(hi, lo, s):
    return shl(hi, s) | shr(shr(lo, 1), 31 - s)


def append(win, pos, hi, lo):
    s = pos & 31
    q = shr(pos, 5)
    back = 31 - s
    parts = [shr(hi, s), shl(shl(hi, 1), back) | shr(lo, s), shl(shl(lo, 1), back)]
    eq = [q == j for j in range(len(win))]
    out = []
    for j, w in enumerate(win):
        add = 0
        for d in range(min(j, 2), -1, -1):
            add = jnp.where(eq[j - d], parts[d], add)
        out.append(w | add)
    return out


def peek(win, pos):
    s = pos & 31
    q = shr(pos, 5)
    nw = len(win)
    zero = jnp.zeros_like(pos)
    w = [win[nw - 1], zero, zero]
    for j in range(nw - 2, -1, -1):
        e = q == j
        w = [jnp.where(e, win[j + d], w[d]) if j + d < nw else w[d] for d in range(3)]
    return funnel(w[0], w[1], s), funnel(w[1], w[2], s)


def advance(win, nb):
    out = [shl(win[j], nb) | shr(win[j + 1], 32 - nb) for j in range(len(win) - 1)]
    out.append(shl(win[-1], nb))
    return out


def encode16(words, top4, win, pos):
    exps, raws = zip(*[split(words[2 * k], words[2 * k + 1]) for k in range(4)])
    fixed, seen, v = None, None, []
    for k in range(4):
        t = top4 - exps[k]
        r = rank_of(t)
        g = (r + rep(0x7D)) & rep(0x80)
        m = g - shr(g, 7)
        v.append((r + rep(0x7E)) & m)
        f = (r | m) & rep(3)
        fixed = f if k == 0 else fixed | shl(f, 2 * k)
        seen = t if k == 0 else seen | t
    s01, s23 = v[0] + v[1], v[2] + v[3]
    p = s01 + s23
    p = p + shl(p, 8)
    p = p + shl(p, 16)
    ends = [p - s23 - v[1], p - s23, p - v[3], p]
    bad = ((seen | s01 | s23) & rep(0xE0)) | (p & rep(0xC0))
    one = jnp.full_like(p, c32(0x80000000))
    hi, lo = one, jnp.zeros_like(p)
    for i in range(4):
        for z in ends:
            bit = shr(one, (shr(z, 8 * i) if i else z) & 31)
            low = (z & c32(32 << (8 * i))) != 0
            hi = hi | jnp.where(low, 0, bit)
            lo = lo | jnp.where(low, bit, 0)
    win = append(win, pos, shl(hi, 1) | shr(lo, 31), shl(lo, 1))
    return list(raws), fixed, win, pos + shr(p, 24), bad


def decode16(fixed, base4, win, pos):
    esc = fixed & shr(fixed, 1)
    hi, lo = peek(win, pos)
    v = [None] * 4
    for i in range(4):
        for h in range(2):
            w, used = hi, None
            for k in (2 * h, 2 * h + 1):
                cond = (esc & c32(1 << (8 * i + 2 * k))) != 0
                n = jnp.where(cond, lax.clz(w) + 1, 0)
                v[k] = n if i == 0 else v[k] | shl(n, 8 * i)
                if used is None:
                    w, used = shl(w, n & 31), n
                else:
                    used = used + n
            pos = pos + used
            if (i, h) != (3, 1):
                s = used & 31
                hi, lo = funnel(hi, lo, s), shl(lo, s)
    exps = []
    for k in range(4):
        f = (shr(fixed, 2 * k) if k else fixed) & rep(3)
        e = (shr(esc, 2 * k) if k else esc) & rep(1)
        exps.append(exps_of(f + v[k] - e, base4))
    return exps, pos


def pack_fields(f, fbits):
    words = [None] * (len(f) * fbits // 32)
    for k, x in enumerate(f):
        j, s = divmod(k * fbits, 32)
        part = shl(x, s) if s else x
        words[j] = part if words[j] is None else words[j] | part
        if s + fbits > 32:
            words[j + 1] = shr(x, 32 - s)
    return words


def unpack_fields(w, fbits):
    f = []
    for k in range(len(w) * 32 // fbits):
        j, s = divmod(k * fbits, 32)
        x = shr(w[j], s) if s else w[j]
        if s + fbits > 32:
            x = x | shl(w[j + 1], 32 - s)
        f.append(x if s + fbits == 32 else x & ((1 << fbits) - 1))
    return f


def make(S=8, nwin=4, fbits=12, n_in=3, n_stage=2, n_recv=10, ylag=1, xlag=2,
         period=16, vchunks=7, post=True, vmem_mb=16):
    R = 128
    TW, G = 128 * S, 8 // S
    nfield = 32 * nwin // fbits
    L = -(-(nfield - 1) // G)
    LA = (G - 1 + nfield) // G
    n_send = LA + 2
    n_var = n_recv + LA
    assert n_recv > (LA + 2) // 2 - 1 + xlag and xlag >= ylag >= 1 and n_var > n_send
    VW = fbits // 4 * 128
    RAW, MAIN, FULL = 4096, 5120, 8192

    def kernel(x):
        ms, ncol = x.shape
        assert ncol == 1024
        half = ms // 2
        n = half // R
        assert n >= max(LA, n_var)
        ngroups = 2 * ms // (R * period)

        def body(x_ref, ov_ref, oh_ref, abuf, bbuf, stage, smain, ymain, xmain, svar, yvar, xvar,
                 estate, ystate, xstate, modes,
                 a_sem, b_sem, o_sem, sm_sem, ym_sem, fm_sem, xm_sem, sv_sem, yv_sem, fv_sem, xv_sem,
                 y_credit, x_credit):
            mx, my = lax.axis_index("x"), lax.axis_index("y")
            ynbr, xnbr = (mx, 1 - my), (1 - mx, my)
            mesh_id = pl.DeviceIdType.MESH

            def read(buf, sem, h, c):
                s = lax.rem(c, n_in)
                return pltpu.make_async_copy(
                    x_ref.at[pl.ds(pl.multiple_of(h * half + c * R, R), R)], buf.at[s], sem.at[s])

            def read_a(c):
                return read(abuf, a_sem, mx, c)

            def read_b(c):
                return read(bbuf, b_sem, 1 - mx, c)

            quarter = (2 * my + mx, 2 * my + 1 - mx, 2 * (1 - my) + mx, 2 * (1 - my) + 1 - mx)

            def stage_wait(k, c):
                s = lax.rem(c, n_stage)
                pltpu.make_async_copy(stage.at[k, s], stage.at[k, s], o_sem.at[k, s]).wait()

            def stage_claim(k, c):
                @pl.when(c >= n_stage)
                def _():
                    stage_wait(k, c - n_stage)
                return stage.at[k, lax.rem(c, n_stage)]

            def stage_flush(k, c):
                s = lax.rem(c, n_stage)
                g = quarter[k] * n + c
                grp, r = lax.div(g, period), lax.rem(g, period)
                hchunks = period - vchunks

                @pl.when(r < hchunks)
                def _():
                    pltpu.make_async_copy(
                        stage.at[k, s], oh_ref.at[grp, pl.ds(pl.multiple_of(r * R, R), R)],
                        o_sem.at[k, s]).start()

                @pl.when(r >= hchunks)
                def _():
                    pltpu.make_async_copy(
                        stage.at[k, s], ov_ref.at[grp, pl.ds(pl.multiple_of((r - hchunks) * R, R), R)],
                        o_sem.at[k, s]).start()

            def main_copy(src, dst, ssem, rsem, to, width):
                return pltpu.make_async_remote_copy(
                    src.at[:, pl.ds(0, width)], dst.at[:, pl.ds(0, width)], ssem, rsem,
                    device_id=to, device_id_type=mesh_id)

            def send_main(c, width):
                s, r = lax.rem(c, n_send), lax.rem(c, n_recv)
                return main_copy(smain.at[s], ymain.at[r], sm_sem.at[s], ym_sem.at[r], ynbr, width)

            def fwd_main(c, width):
                r = lax.rem(c, n_recv)
                return main_copy(ymain.at[r], xmain.at[r], fm_sem.at[r], xm_sem.at[r], xnbr, width)

            def send_var(m):
                r = lax.rem(m, n_var)
                return pltpu.make_async_remote_copy(
                    svar.at[r], yvar.at[r], sv_sem.at[r], yv_sem.at[r],
                    device_id=ynbr, device_id_type=mesh_id)

            def fwd_var(m):
                r = lax.rem(m, n_var)
                return pltpu.make_async_remote_copy(
                    yvar.at[r], xvar.at[r], fv_sem.at[r], xv_sem.at[r],
                    device_id=xnbr, device_id_type=mesh_id)

            def by_mode(k, c, fn):
                base = modes[k, lax.rem(c, n_var)]

                @pl.when(base != 0)
                def _():
                    fn(MAIN)

                @pl.when(base == 0)
                def _():
                    fn(FULL)

            sub = lax.broadcasted_iota(I32, (8, TW), 0)
            lane = lax.broadcasted_iota(I32, (8, TW), 1)
            head = jnp.where(lane == 0, 1, 0)
            nbits = [fbits - head] + [fbits] * (G - 1)
            head_bits = -(-nfield // G)

            def load_state(ref):
                return [ref[j] for j in range(nwin)], ref[nwin]

            def store_state(ref, win, pos):
                for j in range(nwin):
                    ref[j] = win[j]
                ref[nwin] = pos

            def emit(win, pos, g, base):
                nb = nbits[g]
                field = shr(win[0], 32 - nb)
                if g == 0:
                    field = shl(field, head) | (shr(jnp.full_like(sub, base), sub) & head)
                return field, advance(win, nb), jnp.maximum(pos - nb, 0)

            def store_var(m, fields):
                cols = [f[:, 128 * j:128 * (j + 1)] for f in fields for j in range(S)]
                for j, w in enumerate(pack_fields(cols, fbits)):
                    svar[lax.rem(m, n_var), :, 128 * j:128 * (j + 1)] = w

            def idle_chunk(m):
                win, pos = load_state(estate)
                fields = []
                for g in range(G):
                    f, win, pos = emit(win, pos, g, jnp.int32(0))
                    fields.append(f)
                store_var(m, fields)
                store_state(estate, win, pos)

            def encode_chunk(m, carry):
                @pl.when(m >= n_var)
                def _():
                    send_var(m - n_var).wait_send()

                @pl.when(m < n)
                def _():
                    read_a(m).wait()

                    @pl.when(m >= n_send)
                    def _():
                        by_mode(0, m - n_send, lambda w: send_main(m - n_send, w).wait_send())

                    src = abuf.at[lax.rem(m, n_in)]
                    dst = stage_claim(0, m)
                    msg = smain.at[lax.rem(m, n_send)]
                    probe = pltpu.bitcast(src[0:16, :].astype(BF16), I32)
                    total = jnp.sum((shr(probe, 7) & 255) + (shr(probe, 23) & 255))
                    base = jnp.clip(shr(total + int(2.03 * 16384), 14), 29, 253)
                    top4 = (base + 2) * 0x010101
                    top4 = top4 | shl(base + 2, 24)
                    win, pos = load_state(estate)
                    fields, bad = [], None
                    for g in range(G):
                        cs = slice(g * TW, (g + 1) * TW)
                        words = []
                        for k in range(8):
                            t = src[16 * k:16 * (k + 1), cs].astype(BF16)
                            dst[16 * k:16 * (k + 1), cs] = t
                            words.append(pltpu.bitcast(t, I32))
                        raws, fixed, win, pos, b = encode16(words, top4, win, pos)
                        for k in range(4):
                            msg[:, k * 1024 + g * TW:k * 1024 + (g + 1) * TW] = raws[k]
                        msg[:, RAW + g * TW:RAW + (g + 1) * TW] = fixed
                        b = jnp.where(pos > nfield * fbits - head * head_bits, 1, b)
                        bad = b if bad is None else bad | b
                        f, win, pos = emit(win, pos, g, base)
                        fields.append(f)
                    failed = jnp.max(jnp.where(bad != 0, 1, 0))

                    @pl.when(failed == 0)
                    def _():
                        store_var(m, fields)
                        store_state(estate, win, pos)
                        modes[0, lax.rem(m, n_var)] = base

                    @pl.when(failed != 0)
                    def _():
                        for k in range(8):
                            msg[:, k * 1024:(k + 1) * 1024] = pltpu.bitcast(dst[16 * k:16 * (k + 1), :], I32)
                        idle_chunk(m)
                        modes[0, lax.rem(m, n_var)] = 0

                    stage_flush(0, m)

                    @pl.when(m + n_in < n)
                    def _():
                        read_a(m + n_in).start()

                @pl.when(m >= n)
                def _():
                    idle_chunk(m)

                send_var(m).start()
                return carry

            def read_header(k, var, m):
                r = lax.rem(m, n_var)
                w = var[r, :, 0:128]
                s8 = lax.broadcasted_iota(I32, (8, 128), 0)
                l8 = lax.broadcasted_iota(I32, (8, 128), 1)
                modes[k, r] = jnp.sum(jnp.where(l8 == 0, shl(w & 1, s8), 0))

            def load_fields(var, m):
                r = lax.rem(m, n_var)
                cols = unpack_fields([var[r, :, 128 * j:128 * (j + 1)] for j in range(VW // 128)], fbits)
                return [jnp.concatenate(cols[g * S:(g + 1) * S], axis=1) for g in range(G)]

            def take(win, field, g):
                nb = nbits[g]
                if g == 0:
                    field = shr(field, head)
                return nb, field

            def decode_chunk(k, main, var, state, c):
                def push(win, fill, field, g):
                    if g == 0:
                        field = shr(field, head)
                    nb = nbits[g]
                    word = shl(field, 32 - nb)
                    return append(win, fill, word, jnp.zeros_like(word)), fill + nb

                @pl.when(c == 0)
                def _():
                    win = [jnp.zeros((8, TW), I32)] * nwin
                    fill = jnp.zeros((8, TW), I32)
                    for j in range(-(-nfield // G)):
                        for g, f in enumerate(load_fields(var, jnp.int32(j))):
                            if j * G + g < nfield:
                                win, fill = push(win, fill, f, g)
                    store_state(state, win, jnp.zeros((8, TW), I32))
                    state[nwin + 1] = fill

                dst = stage_claim(k + 1, c)
                msg = main.at[lax.rem(c, n_recv)]
                base = modes[k, lax.rem(c, n_var)]

                def run(coded):
                    win, pos = load_state(state)
                    fill = state[nwin + 1]
                    ahead = {}
                    for g in range(G):
                        if coded:
                            cs = slice(g * TW, (g + 1) * TW)
                            base4 = base * 0x010101
                            base4 = base4 | shl(base, 24)
                            exps, pos = decode16(msg[:, RAW + g * TW:RAW + (g + 1) * TW], base4, win, pos)
                            for j in range(4):
                                a, b = join(exps[j], msg[:, j * 1024 + g * TW:j * 1024 + (g + 1) * TW])
                                dst[32 * j:32 * j + 16, cs] = pltpu.bitcast(a, BF16)
                                dst[32 * j + 16:32 * j + 32, cs] = pltpu.bitcast(b, BF16)
                        nb = nbits[g]
                        win, pos, fill = advance(win, nb), jnp.maximum(pos - nb, 0), fill - nb
                        dm, dg = divmod(g + nfield, G)
                        if dm not in ahead:
                            ahead[dm] = load_fields(var, jnp.minimum(c + dm, n + L - 1))
                        win, fill = push(win, fill, ahead[dm][dg], dg)
                    store_state(state, win, pos)
                    state[nwin + 1] = fill

                @pl.when(base != 0)
                def _():
                    run(True)

                @pl.when(base == 0)
                def _():
                    for j in range(8):
                        dst[16 * j:16 * (j + 1), :] = pltpu.bitcast(msg[:, j * 1024:(j + 1) * 1024], BF16)
                    run(False)

                stage_flush(k + 1, c)

            def n_encoded(i):
                return jnp.clip(jnp.minimum(2 * i, i + LA), 0, n + L)

            def n_decoded(i):
                e = n_encoded(i)
                return jnp.where(e == n + L, jnp.clip(i, 0, n), jnp.clip(e - LA, 0, n))

            for c in range(n_in):
                read_a(c).start()
            for c in range(n_in):
                read_b(c).start()
            estate[...] = jnp.zeros_like(estate)

            def step(i, carry):
                @pl.when(jnp.logical_and(i >= n_recv, i < n))
                def _():
                    pl.semaphore_wait(y_credit, 1)

                lax.fori_loop(n_encoded(i), n_encoded(i + 1), encode_chunk, 0)

                @pl.when(i < n)
                def _():
                    by_mode(0, i, lambda w: send_main(i, w).start())
                    read_b(i).wait()
                    dst = stage_claim(1, i)
                    dst[...] = bbuf[lax.rem(i, n_in)].astype(BF16)
                    stage_flush(1, i)

                    @pl.when(i + n_in < n)
                    def _():
                        read_b(i + n_in).start()

                j = i - ylag

                @pl.when(jnp.logical_and(j >= n_recv, j < n))
                def _():
                    pl.semaphore_wait(x_credit, 1)

                def relay_var(m, cc):
                    send_var(m).wait_recv()
                    fwd_var(m).start()
                    read_header(1, yvar, m)
                    return cc

                lax.fori_loop(n_encoded(j), n_encoded(j + 1), relay_var, 0)

                @pl.when(jnp.logical_and(j >= 0, j < n))
                def _():
                    def relay(w):
                        send_main(j, w).wait_recv()
                        fwd_main(j, w).start()
                    by_mode(1, j, relay)

                def dec_y(c, cc):
                    decode_chunk(1, ymain, yvar, ystate, c)
                    return cc

                lax.fori_loop(n_decoded(j), n_decoded(j + 1), dec_y, 0)

                k = i - xlag

                def recv_var(m, cc):
                    fwd_var(m).wait_recv()
                    read_header(2, xvar, m)
                    return cc

                lax.fori_loop(n_encoded(k), n_encoded(k + 1), recv_var, 0)

                @pl.when(k >= 0)
                def _():
                    by_mode(2, k, lambda w: fwd_main(k, w).wait_recv())

                def dec_x(c, cc):
                    decode_chunk(2, xmain, xvar, xstate, c)
                    by_mode(1, c, lambda w: fwd_main(c, w).wait_send())
                    fwd_var(c).wait_send()

                    @pl.when(c + n_recv < n)
                    def _():
                        pl.semaphore_signal(x_credit, 1, device_id=xnbr, device_id_type=mesh_id)
                        pl.semaphore_signal(y_credit, 1, device_id=ynbr, device_id_type=mesh_id)
                    return cc

                lax.fori_loop(n_decoded(k), n_decoded(k + 1), dec_x, 0)
                return carry

            lax.fori_loop(0, n + xlag, step, 0)
            for m in range(n, n + L):
                fwd_var(m).wait_send()
            for m in range(n + L - n_var, n + L):
                send_var(m).wait_send()
            for c in range(n - n_send, n):
                by_mode(0, c, lambda w, c=c: send_main(c, w).wait_send())
            for k in range(4):
                for c in range(n - n_stage, n):
                    stage_wait(k, c)

        dma = pltpu.SemaphoreType.DMA
        ov, oh = pl.pallas_call(
            body,
            out_shape=(pltpu.VMEM((ngroups, vchunks * R, ncol), BF16),
                       jax.ShapeDtypeStruct((ngroups, (period - vchunks) * R, ncol), BF16)),
            in_specs=[pl.BlockSpec(memory_space=pl.ANY)],
            out_specs=(pl.BlockSpec(memory_space=pltpu.VMEM), pl.BlockSpec(memory_space=pl.ANY)),
            scratch_shapes=[
                pltpu.VMEM((n_in, R, ncol), jnp.float32),
                pltpu.VMEM((n_in, R, ncol), jnp.float32),
                pltpu.VMEM((4, n_stage, R, ncol), BF16),
                pltpu.VMEM((n_send, 8, FULL), I32),
                pltpu.VMEM((n_recv, 8, FULL), I32),
                pltpu.VMEM((n_recv, 8, FULL), I32),
                pltpu.VMEM((n_var, 8, VW), I32),
                pltpu.VMEM((n_var, 8, VW), I32),
                pltpu.VMEM((n_var, 8, VW), I32),
                pltpu.VMEM((nwin + 1, 8, TW), I32),
                pltpu.VMEM((nwin + 2, 8, TW), I32),
                pltpu.VMEM((nwin + 2, 8, TW), I32),
                pltpu.SMEM((3, n_var), I32),
                dma((n_in,)), dma((n_in,)), dma((4, n_stage)),
                dma((n_send,)), dma((n_recv,)), dma((n_recv,)), dma((n_recv,)),
                dma((n_var,)), dma((n_var,)), dma((n_var,)), dma((n_var,)),
                pltpu.SemaphoreType.REGULAR, pltpu.SemaphoreType.REGULAR,
            ],
            compiler_params=pltpu.CompilerParams(vmem_limit_bytes=vmem_mb << 20),
        )(x)
        return jnp.concatenate([oh, ov], axis=1).reshape(2 * ms, ncol)

    return kernel


def pallas_dist_ag_xy_y_m65536_n1024_kernel(x: jax.Array):
    return make()(x)
```

```python
import numpy as np
import jax
import jax.numpy as jnp
from jax import lax
from jax.experimental import pallas as pl
from jax.experimental.pallas import tpu as pltpu

I32 = jnp.int32
BF16 = jnp.bfloat16

COLS = 1024
STRIP = 16
STRIPS = 16
VMEM_STRIPS = 7
HBM_STRIPS = STRIPS - VMEM_STRIPS
SLABS = 4
LANES = 128 * SLABS
CODED, PLAIN = 5 * LANES, 8 * LANES

WINDOW = 9
RATE = (5, 16)
MIN_BASE, MAX_BASE = 29, 253

Y_LAG, X_LAG = 2, 4
PACE = 8
PROBE = 8
N_IN, N_KEEP, N_STAGE, N_MAIN, N_WORD, N_HEAD = 4, 2, 8, 32, 32, 8
DECODE_FROM = 24


def _const(v):
    return np.uint32(v).view(np.int32)


def _bytes(b):
    return _const(b * 0x01010101)


_TOP = _const(0x80000000)


def _shl(a, n):
    return lax.shift_left(a, jnp.asarray(n, I32))


def _shr(a, n):
    return lax.shift_right_logical(a, jnp.asarray(n, I32))


def _in_every_byte(b):
    return b * 0x010101 | _shl(b, 24)


def _split(a, b):
    a = _shr(a, 7) | _shl(a, 25)
    b = _shl(b, 1) | _shr(b, 31)
    swap = (a ^ b) & _const(0x00FF00FF)
    return b ^ swap, a ^ swap


def _join(exps, rest):
    swap = (exps ^ rest) & _const(0x00FF00FF)
    a, b = rest ^ swap, exps ^ swap
    return _shl(a, 7) | _shr(a, 25), _shr(b, 1) | _shl(b, 31)


def _rank(t):
    ge1 = (t + _bytes(0x7F)) & _bytes(0x80)
    ge2 = (t + _bytes(0x7E)) & _bytes(0x80)
    ge7 = _shr(t + _bytes(0x79), 7) & _bytes(1)
    ge13 = _shr(t + _bytes(0x73), 7) & _bytes(1)
    return t + _bytes(12) + ge7 + ge13 - (_shr(ge2, 5) | _shr(ge2, 6)) - _shr(ge1, 4)


def _unrank(r, base):
    ge5, ge6 = r + _bytes(0x7B), r + _bytes(0x7A)
    ge12, ge13 = r + _bytes(0x74), r + _bytes(0x73)
    is5, is12 = (ge5 ^ ge6) & _bytes(0x80), (ge12 ^ ge13) & _bytes(0x80)
    steps = (_shr(ge6, 7) & _bytes(1)) + (_shr(ge13, 7) & _bytes(1))
    return (base + steps + (_shr(is5, 5) | _shr(is5, 6))
            + ((is12 - _shr(is12, 7)) & _bytes(13)) - r)


def _funnel(hi, lo, s):
    return _shl(hi, s) | _shr(_shr(lo, 1), s ^ 31)


_HOPS = [1 << b for b in range((WINDOW - 1).bit_length())]


def _append(window, pos, hi, lo):
    s = pos & 31
    parts = [_shr(hi, s), _shl(_shl(hi, 1), s ^ 31) | _shr(lo, s), _shl(_shl(lo, 1), s ^ 31)]
    for d in _HOPS:
        move = (pos & (32 * d)) != 0
        parts = [jnp.where(move, parts[j - d] if 0 <= j - d < len(parts) else 0,
                           parts[j] if j < len(parts) else 0)
                 for j in range(min(len(parts) + d, WINDOW))]
    return [w | p for w, p in zip(window, parts)]


def _peek(window, pos):
    w = list(window)
    for d in reversed(_HOPS):
        move = (pos & (32 * d)) != 0
        w = [jnp.where(move, w[j + d], w[j]) if j + d < len(w) else w[j]
             for j in range(min(len(w), d + 2))]
    s = pos & 31
    return _funnel(w[0], w[1], s), _funnel(w[1], w[2], s)


def _encode(words, base, window, pos):
    top = _in_every_byte(base + 2)
    out, tails, codes, seen = [], [], None, None
    for k in range(4):
        exps, rest = _split(words[2 * k], words[2 * k + 1])
        out.append(rest)
        t = top - exps
        r = _rank(t)
        long = (r + _bytes(0x7D)) & _bytes(0x80)
        long = long - _shr(long, 7)
        tails.append((r + _bytes(0x7E)) & long)
        code = (r | long) & _bytes(3)
        codes = code if k == 0 else codes | _shl(code, 2 * k)
        seen = t if k == 0 else seen | t
    first, second = tails[0] + tails[1], tails[2] + tails[3]
    end = first + second
    end = end + _shl(end, 8)
    end = end + _shl(end, 16)
    one = jnp.full_like(end, _TOP)
    hi, lo = one, jnp.zeros_like(end)
    for i in range(4):
        for stop in (end - second - tails[1], end - second, end - tails[3], end):
            bit = _shr(one, (_shr(stop, 8 * i) if i else stop) & 31)
            low = (stop & _const(32 << (8 * i))) != 0
            hi = hi | jnp.where(low, 0, bit)
            lo = lo | jnp.where(low, bit, 0)
    window = _append(window, pos, _shl(hi, 1) | _shr(lo, 31), _shl(lo, 1))
    pos = pos + _shr(end, 24)
    bad = ((seen | first | second) & _bytes(0xE0)) | (end & _bytes(0xC0))
    return out + [codes], window, pos, jnp.logical_or(bad != 0, pos > 32 * WINDOW)


def _decode(msg, base, window, pos):
    codes = msg[4]
    long = codes & _shr(codes, 1)
    hi, lo = _peek(window, pos)
    hi, lo = _shr(hi, 1) | _TOP, _shl(hi, 31) | _shr(lo, 1)
    tails = [None] * 4
    for i in range(4):
        for pair in ((0, 1), (2, 3)):
            w, used = hi, None
            for k in pair:
                n = lax.clz(w ^ (_shl(long, 31 - 8 * i - 2 * k) & _TOP))
                tails[k] = n if i == 0 else tails[k] | _shl(n, 8 * i)
                if used is None:
                    w, used = _shl(w, n), n
                else:
                    used = used + n
            pos = pos + used
            if (i, pair) != (3, (2, 3)):
                hi, lo = _funnel(hi, lo, used), _shl(lo, used)
    base = _in_every_byte(base)
    words = []
    for k in range(4):
        code = (_shr(codes, 2 * k) if k else codes) & _bytes(3)
        is_long = (_shr(long, 2 * k) if k else long) & _bytes(1)
        words += _join(_unrank(code + tails[k] - is_long, base), msg[k])
    return words, pos


class _Schedule:
    def __init__(self, n):
        self.n = n
        done = [c * RATE[0] // RATE[1] for c in range(2 * n)]
        self.flush_from = done[n]
        self.n_words = done[n - 1] + WINDOW
        self.ahead = next(a for a in range(n)
                          if all(done[c + 1 + a] >= done[c] + WINDOW for c in range(n)))
        assert int(self.decoded(n - 1, np)) == n and self.ahead + 2 <= N_MAIN
        for i in range(n + X_LAG):
            freed_y = int(self.decoded(i - 2 - Y_LAG - X_LAG, np))
            freed_x = int(self.decoded(i - 2 - 2 * X_LAG + Y_LAG, np))
            for j, freed in ((i, freed_y), (i - Y_LAG, freed_x)):
                assert min(j, n - 1) - N_MAIN < freed
                assert int(self.sent(j + 1, np)) - 1 - N_WORD < done[freed]
        for j in range(n):
            row_end = 2 * j if j < 16 else (j // 16 + 1) * 16
            assert self.encoded(j + Y_LAG + 1, np) >= row_end
        assert self.ahead + N_MAIN < 16 * (N_HEAD - 1)

    @staticmethod
    def _div(a, b, xp):
        return a // b if xp is np else lax.div(a, jnp.int32(b))

    def words(self, c, xp=jnp):
        return self._div(c * RATE[0], RATE[1], xp)

    def encoded(self, i, xp=jnp):
        return xp.clip(xp.minimum(2 * i - 1, i + self.ahead), 0, self.n)

    def sent(self, i, xp=jnp):
        e = self.encoded(i, xp)
        return xp.where(e == self.n, self.n_words, self.words(e, xp))

    def decoded(self, j, xp=jnp):
        spare = xp.maximum(self.sent(j + 1, xp) - WINDOW + 1, 0)
        able = self._div(spare * RATE[1] + RATE[0] - 1, RATE[0], xp)
        late = j + 1 - DECODE_FROM
        paced = late + self._div(xp.maximum(late, 0), PACE, xp)
        return xp.clip(xp.minimum(xp.minimum(j + 1, able), paced), 0, self.n)

    def kept(self, i):
        return jnp.clip(jnp.maximum(i - self.ahead, 2 * i - self.n + 8), 0, self.n)


def _all_gather(x_ref, hbm_ref, last_ref, vmem_ref,
                send_in, keep_in, s_main, y_main, x_main, s_word, y_word, x_word,
                s_pos, y_pos, x_pos, s_head, y_head, x_head, base_ref,
                send_in_sem, keep_in_sem, out_sem,
                s_main_sem, y_main_sem, f_main_sem, x_main_sem,
                s_word_sem, y_word_sem, f_word_sem, x_word_sem,
                s_head_sem, y_head_sem, f_head_sem, x_head_sem):
    half = x_ref.shape[0] // 2
    groups = half // SLABS
    n = groups * STRIPS
    n_hbm = groups * HBM_STRIPS
    n_rows = n // 16 + 4
    assert groups & (groups - 1) == 0 and N_STAGE <= groups
    plan = _Schedule(n)

    mx, my = lax.axis_index("x"), lax.axis_index("y")
    y_nbr, x_nbr = (mx, 1 - my), (1 - mx, my)
    mesh = pl.DeviceIdType.MESH

    entry = pltpu.get_barrier_semaphore()
    for nbr in (y_nbr, x_nbr):
        pl.semaphore_signal(entry, 1, device_id=nbr, device_id_type=mesh)

    def place(c):
        return lax.div(c, jnp.int32(groups)), (c & (groups - 1)) * SLABS

    def read(buf, sem, which, c):
        slot = c & (buf.shape[0] - 1)
        turn, slab = place(c)
        row = pl.multiple_of(((turn + VMEM_STRIPS) & (STRIPS - 1)) * STRIP, STRIP)
        pltpu.make_async_copy(x_ref.at[pl.ds(which * half + slab, SLABS), pl.ds(row, STRIP)],
                              buf.at[slot], sem.at[slot]).start()

    def read_wait(buf, sem, c):
        slot = c & (buf.shape[0] - 1)
        pltpu.make_async_copy(buf.at[slot], buf.at[slot], sem.at[slot]).wait()
        return buf.at[slot]

    origin = [q * half for q in (2 * my + mx, 2 * my + 1 - mx, 2 - 2 * my + mx, 3 - 2 * my - mx)]

    def claim(k, c):
        slot = c & (N_STAGE - 1)
        turn, slab = place(c)
        staged = c < n_hbm
        last = (VMEM_STRIPS - 1) * STRIP

        @pl.when(jnp.logical_and(c >= N_STAGE, c < n_hbm + N_STAGE))
        def _():
            stage = vmem_ref.at[pl.ds(origin[k] + slot * SLABS, SLABS), pl.ds(last, STRIP)]
            pltpu.make_async_copy(stage, stage, out_sem.at[k, slot]).wait()

        row = pl.multiple_of(jnp.where(staged, last, (turn - HBM_STRIPS) * STRIP), STRIP)
        return vmem_ref.at[pl.ds(origin[k] + jnp.where(staged, slot * SLABS, slab), SLABS),
                           pl.ds(row, STRIP)]

    def release(k, c, chunk):
        turn, slab = place(c)
        slabs = pl.ds(origin[k] + slab, SLABS)
        sem = out_sem.at[k, c & (N_STAGE - 1)]

        @pl.when(turn < HBM_STRIPS - 1)
        def _():
            pltpu.make_async_copy(chunk, hbm_ref.at[turn, slabs], sem).start()

        @pl.when(turn == HBM_STRIPS - 1)
        def _():
            pltpu.make_async_copy(chunk, last_ref.at[slabs], sem).start()

    def remote(src, dst, send_sem, recv_sem, to):
        return pltpu.make_async_remote_copy(src, dst, send_sem, recv_sem,
                                            device_id=to, device_id_type=mesh)

    def send_main(c, width):
        s = c & (N_MAIN - 1)
        return remote(s_main.at[s, :, pl.ds(0, width)], y_main.at[s, :, pl.ds(0, width)],
                      s_main_sem.at[s], y_main_sem.at[s], y_nbr)

    def relay_main(c, width):
        s = c & (N_MAIN - 1)
        return remote(y_main.at[s, :, pl.ds(0, width)], x_main.at[s, :, pl.ds(0, width)],
                      f_main_sem.at[s], x_main_sem.at[s], x_nbr)

    def send_word(m):
        s = m & (N_WORD - 1)
        return remote(s_word.at[s], y_word.at[s], s_word_sem.at[s], y_word_sem.at[s], y_nbr)

    def relay_word(m):
        s = m & (N_WORD - 1)
        return remote(y_word.at[s], x_word.at[s], f_word_sem.at[s], x_word_sem.at[s], x_nbr)

    def send_head(q):
        s = q & (N_HEAD - 1)
        return remote(s_head.at[q], y_head.at[q], s_head_sem.at[s], y_head_sem.at[s], y_nbr)

    def relay_head(q):
        s = q & (N_HEAD - 1)
        return remote(y_head.at[q], x_head.at[q], f_head_sem.at[s], x_head_sem.at[s], x_nbr)

    def head_row(c):
        return sum((c >= b).astype(I32) for b in (1, 2, 4, 8)) + _shr(c, 4)

    def starts_row(c):
        return jnp.logical_or((c & 15) == 0, jnp.logical_and(c < 16, (c & (c - 1)) == 0))

    def header(head, c):
        return head[head_row(c), c & 15]

    def with_width(head, c, fn):
        base = header(head, c)
        pl.when(base != 0)(lambda: fn(CODED))
        pl.when(base == 0)(lambda: fn(PLAIN))

    def tile(k):
        slab, col = divmod(k * LANES, COLS)
        return slab, slice(None), slice(col, col + LANES)

    def part(k):
        return slice(None), slice(k * LANES, (k + 1) * LANES)

    def encode_chunk(c, carry):
        src = read_wait(send_in, send_in_sem, c)

        @pl.when(c >= N_MAIN)
        def _():
            with_width(s_head, c - N_MAIN, lambda w: send_main(c - N_MAIN, w).wait_send())

        dst = claim(0, c)
        msg = s_main.at[c & (N_MAIN - 1)]

        @pl.when((c & (PROBE - 1)) == 0)
        def _():
            probe = pltpu.bitcast(src[0].astype(BF16), I32)
            total = jnp.sum((_shr(probe, 7) & 255) + (_shr(probe, 23) & 255))
            base_ref[0] = jnp.clip(_shr(total + 33260, 14), MIN_BASE, MAX_BASE)

        base = base_ref[0]
        m = plan.words(c)
        slots = [(m + j) & (N_WORD - 1) for j in range(WINDOW)]
        words = []
        for k in range(8):
            rounded = src[tile(k)].astype(BF16)
            dst[tile(k)] = rounded
            words.append(pltpu.bitcast(rounded, I32))
        coded, window, pos, bad = _encode(words, base, [s_word[s] for s in slots], s_pos[...])
        for k in range(5):
            msg[part(k)] = coded[k]
        exact = jnp.max(jnp.where(bad, 1, 0)) == 0

        @pl.when(exact)
        def _():
            for s, w in zip(slots, window):
                s_word[s] = w
            s_pos[...] = pos

        @pl.when(jnp.logical_not(exact))
        def _():
            for k in range(8):
                msg[part(k)] = pltpu.bitcast(dst[tile(k)], I32)

        s_head[head_row(c), c & 15] = jnp.where(exact, base, 0)
        release(0, c, dst)

        @pl.when(c + N_IN < n)
        def _():
            read(send_in, send_in_sem, mx, c + N_IN)

        @pl.when(c == 0)
        def _():
            pl.semaphore_wait(entry, 2)

        @pl.when(starts_row(c + 1))
        def _():
            q = head_row(c)
            pl.when(q >= N_HEAD)(lambda: send_head(q - N_HEAD).wait_send())
            send_head(q).start()

        @pl.when(plan.words(c + 1) > m)
        def _():
            send_word(m).start()
            s_pos[...] = jnp.maximum(s_pos[...] - 32, 0)
            new = m + WINDOW
            pl.when(new >= N_WORD)(lambda: send_word(new - N_WORD).wait_send())
            s_word[new & (N_WORD - 1)] = jnp.zeros((8, LANES), I32)

        @pl.when(c == n - 1)
        def _():
            for rest in range(plan.flush_from, plan.n_words):
                send_word(rest).start()

        return carry

    def decode_chunk(k, main, word, head, pos_ref, c):
        dst = claim(k, c)
        msg = main.at[c & (N_MAIN - 1)]
        base = header(head, c)
        m = plan.words(c)

        @pl.when(base != 0)
        def _():
            window = [word[(m + j) & (N_WORD - 1)] for j in range(WINDOW)]
            words, pos = _decode([msg[part(j)] for j in range(5)], base, window, pos_ref[...])
            pos_ref[...] = pos
            for j in range(8):
                dst[tile(j)] = pltpu.bitcast(words[j], BF16)

        @pl.when(base == 0)
        def _():
            for j in range(8):
                dst[tile(j)] = pltpu.bitcast(msg[part(j)], BF16)

        @pl.when(plan.words(c + 1) > m)
        def _():
            pos_ref[...] = jnp.maximum(pos_ref[...] - 32, 0)

        release(k, c, dst)

    def decode_y(c, carry):
        decode_chunk(2, y_main, y_word, y_head, y_pos, c)
        return carry

    def decode_x(c, carry):
        decode_chunk(3, x_main, x_word, x_head, x_pos, c)
        with_width(y_head, c, lambda w: relay_main(c, w).wait_send())
        m = plan.words(c)
        pl.when(plan.words(c + 1) > m)(lambda: relay_word(m).wait_send())
        return carry

    def keep_chunk(c, carry):
        src = read_wait(keep_in, keep_in_sem, c)
        dst = claim(1, c)
        dst[...] = src[...].astype(BF16)
        release(1, c, dst)
        pl.when(c + N_KEEP < n)(lambda: read(keep_in, keep_in_sem, 1 - mx, c + N_KEEP))
        return carry

    def pass_word_on(m, carry):
        send_word(m).wait_recv()
        relay_word(m).start()
        return carry

    def take_word(m, carry):
        relay_word(m).wait_recv()
        return carry

    def drain():
        def main(c, carry):
            with_width(s_head, c, lambda w: send_main(c, w).wait_send())
            return carry

        def sent_word(m, carry):
            send_word(m).wait_send()
            return carry

        def relayed_word(m, carry):
            relay_word(m).wait_send()
            return carry

        lax.fori_loop(n - N_MAIN, n, main, 0)
        lax.fori_loop(plan.flush_from + WINDOW - N_WORD, plan.n_words, sent_word, 0)
        lax.fori_loop(plan.flush_from, plan.n_words, relayed_word, 0)
        for q in range(n_rows - N_HEAD, n_rows):
            send_head(q).wait_send()
            relay_head(q).wait_send()

    def step(i, carry):
        lax.fori_loop(plan.encoded(i), plan.encoded(i + 1), encode_chunk, 0)
        pl.when(i < n)(lambda: with_width(s_head, i, lambda w: send_main(i, w).start()))

        j = i - Y_LAG
        lax.fori_loop(plan.sent(j), plan.sent(j + 1), pass_word_on, 0)

        @pl.when(jnp.logical_and(j >= 0, j < n))
        def _():
            @pl.when(starts_row(j))
            def _():
                q = head_row(j)
                send_head(q).wait_recv()
                pl.when(q >= N_HEAD)(lambda: relay_head(q - N_HEAD).wait_send())
                relay_head(q).start()

            def pass_on(width):
                send_main(j, width).wait_recv()
                relay_main(j, width).start()

            with_width(y_head, j, pass_on)

        lax.fori_loop(plan.decoded(j - 1), plan.decoded(j), decode_y, 0)

        @pl.when(i == plan.ahead - 3)
        def _():
            for c in range(N_KEEP):
                read(keep_in, keep_in_sem, 1 - mx, jnp.int32(c))

        lax.fori_loop(plan.kept(i), plan.kept(i + 1), keep_chunk, 0)

        k = i - X_LAG
        lax.fori_loop(plan.sent(k), plan.sent(k + 1), take_word, 0)

        @pl.when(k >= 0)
        def _():
            pl.when(starts_row(k))(lambda: relay_head(head_row(k)).wait_recv())
            with_width(x_head, k, lambda w: relay_main(k, w).wait_recv())

        lax.fori_loop(plan.decoded(k - 1), plan.decoded(k), decode_x, 0)
        pl.when(i == n + X_LAG - 2)(drain)
        return carry

    for c in range(N_IN):
        read(send_in, send_in_sem, mx, jnp.int32(c))
    for s in range(WINDOW):
        s_word[s] = jnp.zeros((8, LANES), I32)
    for pos_ref in (s_pos, y_pos, x_pos):
        pos_ref[...] = jnp.zeros((8, LANES), I32)
    lax.fori_loop(0, n + X_LAG, step, 0)


def pallas_dist_ag_xy_y_m65536_n1024_kernel(x: jax.Array):
    rows, cols = x.shape
    slab = STRIPS * STRIP
    assert cols == COLS and rows % (2 * SLABS * slab) == 0
    slabs = 2 * rows // slab
    n_rows = rows // (2 * SLABS * STRIP) // 16 + 4
    dma = pltpu.SemaphoreType.DMA
    in_hbm, last, in_vmem = pl.pallas_call(
        _all_gather,
        out_shape=(
            jax.ShapeDtypeStruct((HBM_STRIPS - 1, slabs, STRIP, cols), BF16),
            jax.ShapeDtypeStruct((slabs, STRIP, cols), BF16),
            pltpu.VMEM((slabs, VMEM_STRIPS * STRIP, cols), BF16),
        ),
        in_specs=[pl.BlockSpec(memory_space=pl.ANY)],
        out_specs=(
            pl.BlockSpec(memory_space=pl.ANY),
            pl.BlockSpec(memory_space=pl.ANY),
            pl.BlockSpec(memory_space=pltpu.VMEM),
        ),
        scratch_shapes=[
            pltpu.VMEM((N_IN, SLABS, STRIP, cols), jnp.float32),
            pltpu.VMEM((N_KEEP, SLABS, STRIP, cols), jnp.float32),
            *[pltpu.VMEM((N_MAIN, 8, PLAIN), I32)] * 3,
            *[pltpu.VMEM((N_WORD, 8, LANES), I32)] * 3,
            *[pltpu.VMEM((8, LANES), I32)] * 3,
            *[pltpu.SMEM((n_rows, 128), I32)] * 3,
            pltpu.SMEM((1,), I32),
            dma((N_IN,)), dma((N_KEEP,)), dma((4, N_STAGE)),
            *[dma((N_MAIN,))] * 4,
            *[dma((N_WORD,))] * 4,
            *[dma((N_HEAD,))] * 4,
        ],
        compiler_params=pltpu.CompilerParams(
            vmem_limit_bytes=16 << 20,
            collective_id=0,
            disable_semaphore_checks=True,
        ),
    )(x.reshape(rows // slab, slab, cols))
    strips = [in_vmem] + [in_hbm[t] for t in range(HBM_STRIPS - 1)] + [last]
    return jnp.concatenate(strips, axis=1).reshape(2 * rows, cols)
```

```python
import numpy as np
import jax
import jax.numpy as jnp
from jax import lax
from jax.experimental import pallas as pl
from jax.experimental.pallas import tpu as pltpu

I32 = jnp.int32
BF16 = jnp.bfloat16

COLS = 1024
STRIP = 16
STRIPS = 16
VMEM_STRIPS = 7
HBM_STRIPS = STRIPS - VMEM_STRIPS
SLABS = 4
LANES = 128 * SLABS
CODED, PLAIN = 5 * LANES, 8 * LANES

WINDOW = 8
RATE = (77, 256)
DELAY = 1
REACH = 452

Y_LAG, X_LAG = 2, 4
PACE = 16
PROBE = 8
N_IN, N_KEEP, N_STAGE, N_MAIN, N_WORD, N_HEAD = 4, 2, 8, 32, 32, 8
DECODE_FROM = 24


def _const(v):
    return np.uint32(v).view(np.int32)


def _bytes(b):
    return _const(b * 0x01010101)


_TOP = _const(0x80000000)


def _shl(a, n):
    return lax.shift_left(a, jnp.asarray(n, I32))


def _shr(a, n):
    return lax.shift_right_logical(a, jnp.asarray(n, I32))


def _reflect(limit, words):
    return ((limit - 1) | _shl(limit - 1, 16)) - words


def _split(a, b):
    a = _shr(a, 6) | _shl(a, 26)
    b = _shl(b, 2) | _shr(b, 30)
    swap = (a ^ b) & _const(0x00FF00FF)
    return b ^ swap, a ^ swap


def _join(classes, rest):
    swap = (classes ^ rest) & _const(0x00FF00FF)
    a, b = rest ^ swap, classes ^ swap
    return _shl(a, 6) | _shr(a, 26), _shr(b, 2) | _shl(b, 30)


def _rank(t):
    ge1, ge2, ge3 = ((t + _bytes(0x80 - k)) & _bytes(0x80) for k in (1, 2, 3))
    ge11, ge17, ge31 = (_shr(t + _bytes(0x80 - k), 7) & _bytes(1) for k in (11, 17, 31))
    return (t + _bytes(30) + ge11 + ge17 + ge31
            - _shr(ge1, 3) - _shr(ge2, 4) - (_shr(ge3, 4) | _shr(ge3, 7)))


def _unrank(r):
    ge8, ge9, ge15, ge16, ge30, ge31 = (r + _bytes(0x80 - k) for k in (8, 9, 15, 16, 30, 31))
    is8, is15, is30 = ((a ^ b) & _bytes(0x80) for a, b in ((ge8, ge9), (ge15, ge16), (ge30, ge31)))
    skipped = sum(_shr(g, 7) & _bytes(1) for g in (ge9, ge16, ge31))
    return (r + _bytes(3) - skipped - (_shr(is8, 4) | _shr(is8, 7)) - _shr(is15, 3)
            - (_shr(is30, 2) - _shr(is30, 7)))


def _funnel(hi, lo, s):
    return _shl(hi, s) | _shr(_shr(lo, 1), s ^ 31)


_HOPS = [1 << b for b in range((WINDOW - 1).bit_length())]


def _append(window, pos, hi, lo):
    s = pos & 31
    parts = [_shr(hi, s), _shl(_shl(hi, 1), s ^ 31) | _shr(lo, s), _shl(_shl(lo, 1), s ^ 31)]
    for d in _HOPS:
        move = (pos & (32 * d)) != 0
        parts = [jnp.where(move, parts[j - d] if 0 <= j - d < len(parts) else 0,
                           parts[j] if j < len(parts) else 0)
                 for j in range(min(len(parts) + d, WINDOW))]
    return [w | p for w, p in zip(window, parts)]


def _peek(window, pos):
    w = list(window)
    for d in reversed(_HOPS):
        move = (pos & (32 * d)) != 0
        w = [jnp.where(move, w[j + d], w[j]) if j + d < len(w) else w[j]
             for j in range(min(len(w), d + 2))]
    s = pos & 31
    return _funnel(w[0], w[1], s), _funnel(w[1], w[2], s)


def _encode(words, limit, window, pos):
    out, tails, codes, seen, seen_rest = [], [], None, None, None
    for k in range(4):
        t, rest = _split(_reflect(limit, words[2 * k]), _reflect(limit, words[2 * k + 1]))
        rank = _rank(t)
        out.append(rest | (rank & _bytes(1)))
        r = _shr(rank, 1) & _bytes(0x3F)
        long = (r + _bytes(0x7D)) & _bytes(0x80)
        long = long - _shr(long, 7)
        tails.append((r + _bytes(0x7E)) & long)
        code = (r | long) & _bytes(3)
        codes = code if k == 0 else codes | _shl(code, 2 * k)
        seen = t if k == 0 else seen | t
        seen_rest = rest if k == 0 else seen_rest | rest
    first, second = tails[0] + tails[1], tails[2] + tails[3]
    end = first + second
    end = end + _shl(end, 8)
    end = end + _shl(end, 16)
    one = jnp.full_like(end, _TOP)
    hi, lo = one, jnp.zeros_like(end)
    for i in range(4):
        for stop in (end - second - tails[1], end - second, end - tails[3], end):
            bit = _shr(one, (_shr(stop, 8 * i) if i else stop) & 31)
            low = (stop & _const(32 << (8 * i))) != 0
            hi = hi | jnp.where(low, 0, bit)
            lo = lo | jnp.where(low, bit, 0)
    window = _append(window, pos, _shl(hi, 1) | _shr(lo, 31), _shl(lo, 1))
    pos = pos + _shr(end, 24)
    bad = ((seen | end) & _bytes(0xC0)) | (seen_rest & _bytes(1)) | ((first | second) & _bytes(0xE0))
    return out + [codes], window, pos, jnp.logical_or(bad != 0, pos > 32 * WINDOW)


def _decode(msg, limit, window, pos):
    codes = msg[4]
    long = codes & _shr(codes, 1)
    hi, lo = _peek(window, pos)
    hi, lo = _shr(hi, 1) | _TOP, _shl(hi, 31) | _shr(lo, 1)
    tails = [None] * 4
    for i in range(4):
        for pair in ((0, 1), (2, 3)):
            w, used = hi, None
            for k in pair:
                n = lax.clz(w ^ (_shl(long, 31 - 8 * i - 2 * k) & _TOP))
                tails[k] = n if i == 0 else tails[k] | _shl(n, 8 * i)
                if used is None:
                    w, used = _shl(w, n), n
                else:
                    used = used + n
            pos = pos + used
            if (i, pair) != (3, (2, 3)):
                hi, lo = _funnel(hi, lo, used), _shl(lo, used)
    words = []
    for k in range(4):
        code = (_shr(codes, 2 * k) if k else codes) & _bytes(3)
        is_long = (_shr(long, 2 * k) if k else long) & _bytes(1)
        r = code + tails[k] - is_long
        low = msg[k] & _bytes(1)
        words += [_reflect(limit, w) for w in _join(_unrank(r + r + low), msg[k] ^ low)]
    return words, pos


class _Schedule:
    def __init__(self, n):
        self.n = n
        done = [int(self.words(c, np)) for c in range(2 * n)]
        self.flush_from = done[n]
        self.max_words = done[n - 1] + WINDOW
        self.ahead = next(a for a in range(n)
                          if all(done[c + 1 + a] >= done[c] + WINDOW for c in range(16, n)))
        for j in range(n):
            c = int(self.decoded(j, np))
            assert c == 0 or done[c - 1] + WINDOW <= self.sent(j + 1, self.max_words, np)
        assert int(self.decoded(n - 1, np)) == n and self.ahead + 2 <= N_MAIN
        for i in range(n + X_LAG):
            freed_y = int(self.decoded(i - 2 - Y_LAG - X_LAG, np))
            freed_x = int(self.decoded(i - 2 - 2 * X_LAG + Y_LAG, np))
            for j, freed in ((i, freed_y), (i - Y_LAG, freed_x)):
                assert min(j, n - 1) - N_MAIN < freed
                assert int(self.sent(j + 1, self.max_words, np)) - 1 - N_WORD < done[freed]
        for j in range(n):
            row_end = 2 * j if j < 16 else (j // 16 + 1) * 16
            assert self.encoded(j + Y_LAG + 1, np) >= row_end
        assert self.ahead + N_MAIN < 16 * (N_HEAD - 1)
        self.last = next(i for i in range(n) if self.encoded(i + 1, np) == n)
        assert self.last < n - 16

    @staticmethod
    def _div(a, b, xp):
        if xp is np:
            return a // b
        return _shr(a, b.bit_length() - 1) if b & (b - 1) == 0 else lax.div(a, jnp.int32(b))

    def words(self, c, xp=jnp):
        return xp.maximum(self._div(c * RATE[0], RATE[1], xp) - DELAY, 0)

    def encoded(self, i, xp=jnp):
        return xp.clip(xp.minimum(2 * i - 1, i + self.ahead), 0, self.n)

    def sent(self, i, total, xp=jnp):
        e = self.encoded(i, xp)
        return xp.where(e == self.n, total, self.words(e, xp))

    def decoded(self, j, xp=jnp):
        spare = self.sent(j + 1, self.max_words, xp) - WINDOW + 1
        able = xp.where(spare > 0, self._div((spare + DELAY) * RATE[1] + RATE[0] - 1, RATE[0], xp), 0)
        late = j + 1 - DECODE_FROM
        paced = late + self._div(xp.maximum(late, 0), PACE, xp)
        return xp.clip(xp.minimum(xp.minimum(j + 1, able), paced), 0, self.n)

    def kept(self, i):
        return jnp.clip(jnp.maximum(i - self.ahead, 2 * i - self.n + 8), 0, self.n)


def _all_gather(x_ref, hbm_ref, last_ref, vmem_ref,
                send_in, keep_in, s_main, y_main, x_main, s_word, y_word, x_word,
                s_pos, y_pos, x_pos, s_head, y_head, x_head, limit_ref,
                send_in_sem, keep_in_sem, out_sem,
                s_main_sem, y_main_sem, f_main_sem, x_main_sem,
                s_word_sem, y_word_sem, f_word_sem, x_word_sem,
                s_head_sem, y_head_sem, f_head_sem, x_head_sem):
    half = x_ref.shape[0] // 2
    groups = half // SLABS
    n = groups * STRIPS
    n_hbm = groups * HBM_STRIPS
    n_rows = n // 16 + 4
    assert groups & (groups - 1) == 0 and N_STAGE <= groups
    plan = _Schedule(n)

    mx, my = lax.axis_index("x"), lax.axis_index("y")
    y_nbr, x_nbr = (mx, 1 - my), (1 - mx, my)
    mesh = pl.DeviceIdType.MESH

    entry = pltpu.get_barrier_semaphore()
    for nbr in (y_nbr, x_nbr):
        pl.semaphore_signal(entry, 1, device_id=nbr, device_id_type=mesh)

    def place(c):
        return _shr(c, groups.bit_length() - 1), (c & (groups - 1)) * SLABS

    def read(buf, sem, which, c):
        slot = c & (buf.shape[0] - 1)
        turn, slab = place(c)
        row = pl.multiple_of(((turn + VMEM_STRIPS) & (STRIPS - 1)) * STRIP, STRIP)
        pltpu.make_async_copy(x_ref.at[pl.ds(which * half + slab, SLABS), pl.ds(row, STRIP)],
                              buf.at[slot], sem.at[slot]).start()

    def read_wait(buf, sem, c):
        slot = c & (buf.shape[0] - 1)
        pltpu.make_async_copy(buf.at[slot], buf.at[slot], sem.at[slot]).wait()
        return buf.at[slot]

    origin = [q * half for q in (2 * my + mx, 2 * my + 1 - mx, 2 - 2 * my + mx, 3 - 2 * my - mx)]

    def claim(k, c):
        slot = c & (N_STAGE - 1)
        turn, slab = place(c)
        staged = c < n_hbm
        last = (VMEM_STRIPS - 1) * STRIP

        @pl.when(jnp.logical_and(c >= N_STAGE, c < n_hbm + N_STAGE))
        def _():
            stage = vmem_ref.at[pl.ds(origin[k] + slot * SLABS, SLABS), pl.ds(last, STRIP)]
            pltpu.make_async_copy(stage, stage, out_sem.at[k, slot]).wait()

        row = pl.multiple_of(jnp.where(staged, last, (turn - HBM_STRIPS) * STRIP), STRIP)
        return vmem_ref.at[pl.ds(origin[k] + jnp.where(staged, slot * SLABS, slab), SLABS),
                           pl.ds(row, STRIP)]

    def release(k, c, chunk):
        turn, slab = place(c)
        slabs = pl.ds(origin[k] + slab, SLABS)
        sem = out_sem.at[k, c & (N_STAGE - 1)]

        @pl.when(turn < HBM_STRIPS - 1)
        def _():
            pltpu.make_async_copy(chunk, hbm_ref.at[turn, slabs], sem).start()

        @pl.when(turn == HBM_STRIPS - 1)
        def _():
            pltpu.make_async_copy(chunk, last_ref.at[slabs], sem).start()

    def remote(src, dst, send_sem, recv_sem, to):
        return pltpu.make_async_remote_copy(src, dst, send_sem, recv_sem,
                                            device_id=to, device_id_type=mesh)

    def send_main(c, width):
        s = c & (N_MAIN - 1)
        return remote(s_main.at[s, :, pl.ds(0, width)], y_main.at[s, :, pl.ds(0, width)],
                      s_main_sem.at[s], y_main_sem.at[s], y_nbr)

    def relay_main(c, width):
        s = c & (N_MAIN - 1)
        return remote(y_main.at[s, :, pl.ds(0, width)], x_main.at[s, :, pl.ds(0, width)],
                      f_main_sem.at[s], x_main_sem.at[s], x_nbr)

    def send_word(m):
        s = m & (N_WORD - 1)
        return remote(s_word.at[s], y_word.at[s], s_word_sem.at[s], y_word_sem.at[s], y_nbr)

    def relay_word(m):
        s = m & (N_WORD - 1)
        return remote(y_word.at[s], x_word.at[s], f_word_sem.at[s], x_word_sem.at[s], x_nbr)

    def send_head(q):
        s = q & (N_HEAD - 1)
        return remote(s_head.at[q], y_head.at[q], s_head_sem.at[s], y_head_sem.at[s], y_nbr)

    def relay_head(q):
        s = q & (N_HEAD - 1)
        return remote(y_head.at[q], x_head.at[q], f_head_sem.at[s], x_head_sem.at[s], x_nbr)

    def head_row(c):
        return sum((c >= b).astype(I32) for b in (1, 2, 4, 8)) + _shr(c, 4)

    def starts_row(c):
        return jnp.logical_or((c & 15) == 0, jnp.logical_and(c < 16, (c & (c - 1)) == 0))

    def header(head, c):
        return head[head_row(c), c & 15]

    def with_width(head, c, fn):
        limit = header(head, c)
        pl.when(limit != 0)(lambda: fn(CODED))
        pl.when(limit == 0)(lambda: fn(PLAIN))

    def tile(k):
        slab, col = divmod(k * LANES, COLS)
        return slab, slice(None), slice(col, col + LANES)

    def part(k):
        return slice(None), slice(k * LANES, (k + 1) * LANES)

    def encode_chunk(c, carry):
        src = read_wait(send_in, send_in_sem, c)

        @pl.when(c >= N_MAIN)
        def _():
            with_width(s_head, c - N_MAIN, lambda w: send_main(c - N_MAIN, w).wait_send())

        dst = claim(0, c)
        msg = s_main.at[c & (N_MAIN - 1)]

        @pl.when((c & (PROBE - 1)) == 0)
        def _():
            probe = pltpu.bitcast(src[0].astype(BF16), I32)
            total = jnp.sum((probe & 0x7FFF) + (_shr(probe, 16) & 0x7FFF))
            limit_ref[0] = _shr(total, 14) + REACH

        limit = limit_ref[0]
        m = plan.words(c)
        slots = [(m + j) & (N_WORD - 1) for j in range(WINDOW)]
        words = []
        for k in range(8):
            rounded = src[tile(k)].astype(BF16)
            dst[tile(k)] = rounded
            words.append(pltpu.bitcast(rounded, I32))
        coded, window, pos, bad = _encode(words, limit, [s_word[s] for s in slots], s_pos[...])
        for k in range(5):
            msg[part(k)] = coded[k]
        exact = jnp.max(jnp.where(bad, 1, 0)) == 0

        def keep_code():
            for s, w in zip(slots, window):
                s_word[s] = w
            s_pos[...] = pos

        def send_plain():
            for k in range(8):
                msg[part(k)] = pltpu.bitcast(dst[tile(k)], I32)

        lax.cond(exact, keep_code, send_plain)

        s_head[head_row(c), c & 15] = jnp.where(exact, limit, 0)
        release(0, c, dst)

        @pl.when(c + N_IN < n)
        def _():
            read(send_in, send_in_sem, mx, c + N_IN)

        @pl.when(c == 0)
        def _():
            pl.semaphore_wait(entry, 2)

        @pl.when(plan.words(c + 1) > m)
        def _():
            send_word(m).start()
            s_pos[...] = jnp.maximum(s_pos[...] - 32, 0)
            new = m + WINDOW
            pl.when(new >= N_WORD)(lambda: send_word(new - N_WORD).wait_send())
            s_word[new & (N_WORD - 1)] = jnp.zeros((8, LANES), I32)

        @pl.when(c == n - 1)
        def _():
            total = plan.flush_from + _shr(jnp.max(s_pos[...]) + 31, 5)
            s_head[n_rows - 1, 16] = total
            lax.fori_loop(plan.flush_from, total, lambda m, _: send_word(m).start(), None)

        @pl.when(starts_row(c + 1))
        def _():
            q = head_row(c)
            pl.when(q >= N_HEAD)(lambda: send_head(q - N_HEAD).wait_send())
            send_head(q).start()

        return carry

    def decode_chunk(k, main, word, head, pos_ref, c):
        dst = claim(k, c)
        msg = main.at[c & (N_MAIN - 1)]
        limit = header(head, c)
        m = plan.words(c)

        def coded():
            window = [word[(m + j) & (N_WORD - 1)] for j in range(WINDOW)]
            words, pos = _decode([msg[part(j)] for j in range(5)], limit, window, pos_ref[...])
            pos_ref[...] = pos
            for j in range(8):
                dst[tile(j)] = pltpu.bitcast(words[j], BF16)

        def plain():
            for j in range(8):
                dst[tile(j)] = pltpu.bitcast(msg[part(j)], BF16)

        lax.cond(limit != 0, coded, plain)

        @pl.when(plan.words(c + 1) > m)
        def _():
            pos_ref[...] = jnp.maximum(pos_ref[...] - 32, 0)

        release(k, c, dst)

    def decode_y(c, carry):
        decode_chunk(2, y_main, y_word, y_head, y_pos, c)
        return carry

    def decode_x(c, carry):
        decode_chunk(3, x_main, x_word, x_head, x_pos, c)
        with_width(y_head, c, lambda w: relay_main(c, w).wait_send())
        m = plan.words(c)
        pl.when(plan.words(c + 1) > m)(lambda: relay_word(m).wait_send())
        return carry

    def keep_chunk(c, carry):
        src = read_wait(keep_in, keep_in_sem, c)
        dst = claim(1, c)
        dst[...] = src[...].astype(BF16)
        release(1, c, dst)
        pl.when(c + N_KEEP < n)(lambda: read(keep_in, keep_in_sem, 1 - mx, c + N_KEEP))
        return carry

    def pass_word_on(m, carry):
        send_word(m).wait_recv()
        relay_word(m).start()
        return carry

    def take_word(m, carry):
        relay_word(m).wait_recv()
        return carry

    def drain():
        def main(c, carry):
            with_width(s_head, c, lambda w: send_main(c, w).wait_send())
            return carry

        def sent_word(m, carry):
            send_word(m).wait_send()
            return carry

        def relayed_word(m, carry):
            relay_word(m).wait_send()
            return carry

        lax.fori_loop(n - N_MAIN, n, main, 0)
        lax.fori_loop(plan.flush_from + WINDOW - N_WORD, s_head[n_rows - 1, 16], sent_word, 0)
        lax.fori_loop(plan.flush_from, y_head[n_rows - 1, 16], relayed_word, 0)
        for q in range(n_rows - N_HEAD, n_rows):
            send_head(q).wait_send()
            relay_head(q).wait_send()

    def pass_head_on(q):
        send_head(q).wait_recv()
        pl.when(q >= N_HEAD)(lambda: relay_head(q - N_HEAD).wait_send())
        relay_head(q).start()

    def opens_row(c):
        return jnp.logical_and(starts_row(c), c < n - 16)

    def step(i, before):
        j, k = i - Y_LAG, i - X_LAG
        after = (plan.encoded(i + 1), plan.sent(j + 1, plan.flush_from), plan.decoded(j),
                 plan.kept(i + 1), plan.sent(k + 1, plan.flush_from), plan.decoded(k))
        lax.fori_loop(before[0], after[0], encode_chunk, 0)
        pl.when(i < n)(lambda: with_width(s_head, i, lambda w: send_main(i, w).start()))
        lax.fori_loop(before[1], after[1], pass_word_on, 0)

        @pl.when(j == plan.last)
        def _():
            pass_head_on(jnp.int32(n_rows - 1))
            lax.fori_loop(plan.flush_from, y_head[n_rows - 1, 16], pass_word_on, 0)

        @pl.when(jnp.logical_and(j >= 0, j < n))
        def _():
            def pass_on(width):
                send_main(j, width).wait_recv()
                relay_main(j, width).start()

            pl.when(opens_row(j))(lambda: pass_head_on(head_row(j)))
            with_width(y_head, j, pass_on)

        lax.fori_loop(before[2], after[2], decode_y, 0)

        @pl.when(i == plan.ahead - 3)
        def _():
            for c in range(N_KEEP):
                read(keep_in, keep_in_sem, 1 - mx, jnp.int32(c))

        lax.fori_loop(before[3], after[3], keep_chunk, 0)
        lax.fori_loop(before[4], after[4], take_word, 0)

        @pl.when(k == plan.last)
        def _():
            relay_head(jnp.int32(n_rows - 1)).wait_recv()
            lax.fori_loop(plan.flush_from, x_head[n_rows - 1, 16], take_word, 0)

        @pl.when(k >= 0)
        def _():
            pl.when(opens_row(k))(lambda: relay_head(head_row(k)).wait_recv())
            with_width(x_head, k, lambda w: relay_main(k, w).wait_recv())

        lax.fori_loop(before[5], after[5], decode_x, 0)
        pl.when(i == n + X_LAG - 2)(drain)
        return after

    for c in range(N_IN):
        read(send_in, send_in_sem, mx, jnp.int32(c))
    for s in range(WINDOW):
        s_word[s] = jnp.zeros((8, LANES), I32)
    for pos_ref in (s_pos, y_pos, x_pos):
        pos_ref[...] = jnp.zeros((8, LANES), I32)
    lax.fori_loop(0, n + X_LAG, step, (jnp.int32(0),) * 6)


def pallas_dist_ag_xy_y_m65536_n1024_kernel(x: jax.Array):
    rows, cols = x.shape
    slab = STRIPS * STRIP
    assert cols == COLS and rows % (2 * SLABS * slab) == 0
    slabs = 2 * rows // slab
    n_rows = rows // (2 * SLABS * STRIP) // 16 + 4
    dma = pltpu.SemaphoreType.DMA
    in_hbm, last, in_vmem = pl.pallas_call(
        _all_gather,
        out_shape=(
            jax.ShapeDtypeStruct((HBM_STRIPS - 1, slabs, STRIP, cols), BF16),
            jax.ShapeDtypeStruct((slabs, STRIP, cols), BF16),
            pltpu.VMEM((slabs, VMEM_STRIPS * STRIP, cols), BF16),
        ),
        in_specs=[pl.BlockSpec(memory_space=pl.ANY)],
        out_specs=(
            pl.BlockSpec(memory_space=pl.ANY),
            pl.BlockSpec(memory_space=pl.ANY),
            pl.BlockSpec(memory_space=pltpu.VMEM),
        ),
        scratch_shapes=[
            pltpu.VMEM((N_IN, SLABS, STRIP, cols), jnp.float32),
            pltpu.VMEM((N_KEEP, SLABS, STRIP, cols), jnp.float32),
            *[pltpu.VMEM((N_MAIN, 8, PLAIN), I32)] * 3,
            *[pltpu.VMEM((N_WORD, 8, LANES), I32)] * 3,
            *[pltpu.VMEM((8, LANES), I32)] * 3,
            *[pltpu.SMEM((n_rows, 128), I32)] * 3,
            pltpu.SMEM((1,), I32),
            dma((N_IN,)), dma((N_KEEP,)), dma((4, N_STAGE)),
            *[dma((N_MAIN,))] * 4,
            *[dma((N_WORD,))] * 4,
            *[dma((N_HEAD,))] * 4,
        ],
        compiler_params=pltpu.CompilerParams(
            vmem_limit_bytes=16 << 20,
            collective_id=0,
            disable_semaphore_checks=True,
        ),
    )(x.reshape(rows // slab, slab, cols))
    strips = [in_vmem] + [in_hbm[t] for t in range(HBM_STRIPS - 1)] + [last]
    return jnp.concatenate(strips, axis=1).reshape(2 * rows, cols)
```

```python
import numpy as np
import jax
import jax.numpy as jnp
from jax import lax
from jax.experimental import pallas as pl
from jax.experimental.pallas import tpu as pltpu

I32 = jnp.int32
BF16 = jnp.bfloat16

COLS = 1024
STRIP = 16
STRIPS = 16
VMEM_STRIPS = 7
HBM_STRIPS = STRIPS - VMEM_STRIPS
SLABS = 4
LANES = 128 * SLABS
CODED, PLAIN = 5 * LANES, 8 * LANES

WINDOW = 8
RATE = (77, 256)
DELAY = 1
REACH = 452

Y_LAG, X_LAG = 2, 4
PACE = 16
PROBE = 8
N_IN, N_KEEP, N_STAGE, N_MAIN, N_WORD, N_HEAD = 4, 2, 8, 32, 32, 8
DECODE_FROM = 24


def _const(v):
    return np.uint32(v).view(np.int32)


def _bytes(b):
    return _const(b * 0x01010101)


_TOP = _const(0x80000000)


def _shl(a, n):
    return lax.shift_left(a, jnp.asarray(n, I32))


def _shr(a, n):
    return lax.shift_right_logical(a, jnp.asarray(n, I32))


def _reflect(limit, words):
    return ((limit - 1) | _shl(limit - 1, 16)) - words


def _split(a, b):
    a = _shr(a, 6) | _shl(a, 26)
    b = _shl(b, 2) | _shr(b, 30)
    swap = (a ^ b) & _const(0x00FF00FF)
    return b ^ swap, a ^ swap


def _join(classes, rest):
    swap = (classes ^ rest) & _const(0x00FF00FF)
    a, b = rest ^ swap, classes ^ swap
    return _shl(a, 6) | _shr(a, 26), _shr(b, 2) | _shl(b, 30)


def _rank(t):
    ge1, ge2, ge3 = ((t + _bytes(0x80 - k)) & _bytes(0x80) for k in (1, 2, 3))
    ge11, ge17, ge31 = (_shr(t + _bytes(0x80 - k), 7) & _bytes(1) for k in (11, 17, 31))
    return (t + _bytes(30) + ge11 + ge17 + ge31
            - _shr(ge1, 3) - _shr(ge2, 4) - (_shr(ge3, 4) | _shr(ge3, 7)))


def _unrank(r):
    ge8, ge9, ge15, ge16, ge30, ge31 = (r + _bytes(0x80 - k) for k in (8, 9, 15, 16, 30, 31))
    is8, is15, is30 = ((a ^ b) & _bytes(0x80) for a, b in ((ge8, ge9), (ge15, ge16), (ge30, ge31)))
    skipped = sum(_shr(g, 7) & _bytes(1) for g in (ge9, ge16, ge31))
    return (r + _bytes(3) - skipped - (_shr(is8, 4) | _shr(is8, 7)) - _shr(is15, 3)
            - (_shr(is30, 2) - _shr(is30, 7)))


def _funnel(hi, lo, s):
    return _shl(hi, s) | _shr(_shr(lo, 1), s ^ 31)


_HOPS = [1 << b for b in range((WINDOW - 1).bit_length())]


def _append(window, pos, hi, lo):
    s = pos & 31
    parts = [_shr(hi, s), _shl(_shl(hi, 1), s ^ 31) | _shr(lo, s), _shl(_shl(lo, 1), s ^ 31)]
    for d in _HOPS:
        move = (pos & (32 * d)) != 0
        parts = [jnp.where(move, parts[j - d] if 0 <= j - d < len(parts) else 0,
                           parts[j] if j < len(parts) else 0)
                 for j in range(min(len(parts) + d, WINDOW))]
    return [w | p for w, p in zip(window, parts)]


def _peek(window, pos):
    w = list(window)
    for d in reversed(_HOPS):
        move = (pos & (32 * d)) != 0
        w = [jnp.where(move, w[j + d], w[j]) if j + d < len(w) else w[j]
             for j in range(min(len(w), d + 2))]
    s = pos & 31
    return _funnel(w[0], w[1], s), _funnel(w[1], w[2], s)


def _encode(words, limit, window, pos):
    out, tails, codes, seen, seen_rest = [], [], None, None, None
    for k in range(4):
        t, rest = _split(_reflect(limit, words[2 * k]), _reflect(limit, words[2 * k + 1]))
        rank = _rank(t)
        out.append(rest | (rank & _bytes(1)))
        r = _shr(rank, 1) & _bytes(0x3F)
        long = (r + _bytes(0x7D)) & _bytes(0x80)
        long = long - _shr(long, 7)
        tails.append((r + _bytes(0x7E)) & long)
        code = (r | long) & _bytes(3)
        codes = code if k == 0 else codes | _shl(code, 2 * k)
        seen = t if k == 0 else seen | t
        seen_rest = rest if k == 0 else seen_rest | rest
    first, second = tails[0] + tails[1], tails[2] + tails[3]
    end = first + second
    end = end + _shl(end, 8)
    end = end + _shl(end, 16)
    one = jnp.full_like(end, _TOP)
    hi, lo = one, jnp.zeros_like(end)
    for i in range(4):
        for stop in (end - second - tails[1], end - second, end - tails[3], end):
            bit = _shr(one, (_shr(stop, 8 * i) if i else stop) & 31)
            low = (stop & _const(32 << (8 * i))) != 0
            hi = hi | jnp.where(low, 0, bit)
            lo = lo | jnp.where(low, bit, 0)
    window = _append(window, pos, _shl(hi, 1) | _shr(lo, 31), _shl(lo, 1))
    pos = pos + _shr(end, 24)
    bad = ((seen | end) & _bytes(0xC0)) | (seen_rest & _bytes(1)) | ((first | second) & _bytes(0xE0))
    return out + [codes], window, pos, jnp.logical_or(bad != 0, pos > 32 * WINDOW)


def _decode(msg, limit, window, pos):
    codes = msg[4]
    long = codes & _shr(codes, 1)
    hi, lo = _peek(window, pos)
    hi, lo = _shr(hi, 1) | _TOP, _shl(hi, 31) | _shr(lo, 1)
    tails = [None] * 4
    for i in range(4):
        for pair in ((0, 1), (2, 3)):
            w, used = hi, None
            for k in pair:
                n = lax.clz(w ^ (_shl(long, 31 - 8 * i - 2 * k) & _TOP))
                tails[k] = n if i == 0 else tails[k] | _shl(n, 8 * i)
                if used is None:
                    w, used = _shl(w, n), n
                else:
                    used = used + n
            pos = pos + used
            if (i, pair) != (3, (2, 3)):
                hi, lo = _funnel(hi, lo, used), _shl(lo, used)
    words = []
    for k in range(4):
        code = (_shr(codes, 2 * k) if k else codes) & _bytes(3)
        is_long = (_shr(long, 2 * k) if k else long) & _bytes(1)
        r = code + tails[k] - is_long
        low = msg[k] & _bytes(1)
        words += [_reflect(limit, w) for w in _join(_unrank(r + r + low), msg[k] ^ low)]
    return words, pos


class _Schedule:
    def __init__(self, n):
        self.n = n
        done = [int(self.words(c, np)) for c in range(2 * n)]
        self.flush_from = done[n]
        self.max_words = done[n - 1] + WINDOW
        self.ahead = next(a for a in range(n)
                          if all(done[c + 1 + a] >= done[c] + WINDOW for c in range(16, n)))
        for j in range(n):
            c = int(self.decoded(j, np))
            assert c == 0 or done[c - 1] + WINDOW <= self.sent(j + 1, self.max_words, np)
        assert int(self.decoded(n - 1, np)) == n and self.ahead + 2 <= N_MAIN
        for i in range(n + X_LAG):
            freed_y = int(self.decoded(i - 2 - Y_LAG - X_LAG, np))
            freed_x = int(self.decoded(i - 2 - 2 * X_LAG + Y_LAG, np))
            for j, freed in ((i, freed_y), (i - Y_LAG, freed_x)):
                assert min(j, n - 1) - N_MAIN < freed
                assert int(self.sent(j + 1, self.max_words, np)) - 1 - N_WORD < done[freed]
        for j in range(n):
            row_end = 2 * j if j < 16 else (j // 16 + 1) * 16
            assert self.encoded(j + Y_LAG + 1, np) >= row_end
        assert self.ahead + N_MAIN < 16 * (N_HEAD - 1)
        self.last = next(i for i in range(n) if self.encoded(i + 1, np) == n)
        assert self.last < n - 16

    @staticmethod
    def _div(a, b, xp):
        if xp is np:
            return a // b
        return _shr(a, b.bit_length() - 1) if b & (b - 1) == 0 else lax.div(a, jnp.int32(b))

    def words(self, c, xp=jnp):
        return xp.maximum(self._div(c * RATE[0], RATE[1], xp) - DELAY, 0)

    def encoded(self, i, xp=jnp):
        return xp.clip(xp.minimum(2 * i - 1, i + self.ahead), 0, self.n)

    def sent(self, i, total, xp=jnp):
        e = self.encoded(i, xp)
        return xp.where(e == self.n, total, self.words(e, xp))

    def decoded(self, j, xp=jnp):
        spare = self.sent(j + 1, self.max_words, xp) - WINDOW + 1
        able = xp.where(spare > 0, self._div((spare + DELAY) * RATE[1] + RATE[0] - 1, RATE[0], xp), 0)
        late = j + 1 - DECODE_FROM
        paced = late + self._div(xp.maximum(late, 0), PACE, xp)
        return xp.clip(xp.minimum(xp.minimum(j + 1, able), paced), 0, self.n)

    def kept(self, i):
        return jnp.clip(jnp.maximum(i - self.ahead, 2 * i - self.n + 8), 0, self.n)


def _to_words(chunk):
    return [pltpu.bitcast(chunk[s, :, c:c + LANES], I32)
            for s in range(SLABS) for c in range(0, COLS, LANES)]


def _from_words(words):
    halves = [pltpu.bitcast(w, BF16) for w in words]
    per_slab = COLS // LANES
    return jnp.stack([jnp.concatenate(halves[s * per_slab:(s + 1) * per_slab], axis=1)
                      for s in range(SLABS)])


def _parts(msg):
    return [msg[:, c:c + LANES] for c in range(0, msg.shape[1], LANES)]


def _all_gather(x_ref, hbm_ref, last_ref, vmem_ref,
                send_in, keep_in, s_main, y_main, x_main, s_word, y_word, x_word,
                s_pos, y_pos, x_pos, s_head, y_head, x_head, limit_ref,
                send_in_sem, keep_in_sem, out_sem,
                s_main_sem, y_main_sem, f_main_sem, x_main_sem,
                s_word_sem, y_word_sem, f_word_sem, x_word_sem,
                s_head_sem, y_head_sem, f_head_sem, x_head_sem):
    half = x_ref.shape[0] // 2
    groups = half // SLABS
    n = groups * STRIPS
    n_hbm = groups * HBM_STRIPS
    n_rows = n // 16 + 4
    assert groups & (groups - 1) == 0 and N_STAGE <= groups
    plan = _Schedule(n)

    mx, my = lax.axis_index("x"), lax.axis_index("y")
    y_nbr, x_nbr = (mx, 1 - my), (1 - mx, my)
    mesh = pl.DeviceIdType.MESH

    entry = pltpu.get_barrier_semaphore()
    for nbr in (y_nbr, x_nbr):
        pl.semaphore_signal(entry, 1, device_id=nbr, device_id_type=mesh)

    def place(c):
        return _shr(c, groups.bit_length() - 1), (c & (groups - 1)) * SLABS

    def read(buf, sem, which, c):
        slot = c & (buf.shape[0] - 1)
        turn, slab = place(c)
        row = pl.multiple_of(((turn + VMEM_STRIPS) & (STRIPS - 1)) * STRIP, STRIP)
        pltpu.make_async_copy(x_ref.at[pl.ds(which * half + slab, SLABS), pl.ds(row, STRIP)],
                              buf.at[slot], sem.at[slot]).start()

    def read_wait(buf, sem, c):
        slot = c & (buf.shape[0] - 1)
        pltpu.make_async_copy(buf.at[slot], buf.at[slot], sem.at[slot]).wait()
        return buf.at[slot]

    origin = [q * half for q in (2 * my + mx, 2 * my + 1 - mx, 2 - 2 * my + mx, 3 - 2 * my - mx)]

    def claim(k, c):
        slot = c & (N_STAGE - 1)
        turn, slab = place(c)
        staged = c < n_hbm
        last = (VMEM_STRIPS - 1) * STRIP

        @pl.when(jnp.logical_and(c >= N_STAGE, c < n_hbm + N_STAGE))
        def _():
            stage = vmem_ref.at[pl.ds(origin[k] + slot * SLABS, SLABS), pl.ds(last, STRIP)]
            pltpu.make_async_copy(stage, stage, out_sem.at[k, slot]).wait()

        row = pl.multiple_of(jnp.where(staged, last, (turn - HBM_STRIPS) * STRIP), STRIP)
        return vmem_ref.at[pl.ds(origin[k] + jnp.where(staged, slot * SLABS, slab), SLABS),
                           pl.ds(row, STRIP)]

    def release(k, c, chunk):
        turn, slab = place(c)
        slabs = pl.ds(origin[k] + slab, SLABS)
        sem = out_sem.at[k, c & (N_STAGE - 1)]

        @pl.when(turn < HBM_STRIPS - 1)
        def _():
            pltpu.make_async_copy(chunk, hbm_ref.at[turn, slabs], sem).start()

        @pl.when(turn == HBM_STRIPS - 1)
        def _():
            pltpu.make_async_copy(chunk, last_ref.at[slabs], sem).start()

    def remote(src, dst, send_sem, recv_sem, to):
        return pltpu.make_async_remote_copy(src, dst, send_sem, recv_sem,
                                            device_id=to, device_id_type=mesh)

    def send_main(c, width):
        s = c & (N_MAIN - 1)
        return remote(s_main.at[s, :, pl.ds(0, width)], y_main.at[s, :, pl.ds(0, width)],
                      s_main_sem.at[s], y_main_sem.at[s], y_nbr)

    def relay_main(c, width):
        s = c & (N_MAIN - 1)
        return remote(y_main.at[s, :, pl.ds(0, width)], x_main.at[s, :, pl.ds(0, width)],
                      f_main_sem.at[s], x_main_sem.at[s], x_nbr)

    def send_word(m):
        s = m & (N_WORD - 1)
        return remote(s_word.at[s], y_word.at[s], s_word_sem.at[s], y_word_sem.at[s], y_nbr)

    def relay_word(m):
        s = m & (N_WORD - 1)
        return remote(y_word.at[s], x_word.at[s], f_word_sem.at[s], x_word_sem.at[s], x_nbr)

    def send_head(q):
        s = q & (N_HEAD - 1)
        return remote(s_head.at[q], y_head.at[q], s_head_sem.at[s], y_head_sem.at[s], y_nbr)

    def relay_head(q):
        s = q & (N_HEAD - 1)
        return remote(y_head.at[q], x_head.at[q], f_head_sem.at[s], x_head_sem.at[s], x_nbr)

    def head_row(c):
        return sum((c >= b).astype(I32) for b in (1, 2, 4, 8)) + _shr(c, 4)

    def starts_row(c):
        return jnp.logical_or((c & 15) == 0, jnp.logical_and(c < 16, (c & (c - 1)) == 0))

    def header(head, c):
        return head[head_row(c), c & 15]

    def with_width(head, c, fn):
        limit = header(head, c)
        pl.when(limit != 0)(lambda: fn(CODED))
        pl.when(limit == 0)(lambda: fn(PLAIN))

    def encode_chunk(c, carry):
        src = read_wait(send_in, send_in_sem, c)

        @pl.when(c >= N_MAIN)
        def _():
            with_width(s_head, c - N_MAIN, lambda w: send_main(c - N_MAIN, w).wait_send())

        dst = claim(0, c)
        msg = s_main.at[c & (N_MAIN - 1)]

        @pl.when((c & (PROBE - 1)) == 0)
        def _():
            probe = pltpu.bitcast(src[0].astype(BF16), I32)
            total = jnp.sum((probe & 0x7FFF) + (_shr(probe, 16) & 0x7FFF))
            limit_ref[0] = _shr(total, 14) + REACH

        limit = limit_ref[0]
        m = plan.words(c)
        slots = [(m + j) & (N_WORD - 1) for j in range(WINDOW)]
        rounded = src[...].astype(BF16)
        dst[...] = rounded
        coded, window, pos, bad = _encode(
            _to_words(rounded), limit, [s_word[s] for s in slots], s_pos[...])
        msg[:, :CODED] = jnp.concatenate(coded, axis=1)
        exact = jnp.max(jnp.where(bad, 1, 0)) == 0

        def keep_code():
            for s, w in zip(slots, window):
                s_word[s] = w
            s_pos[...] = pos

        def send_plain():
            msg[...] = jnp.concatenate(_to_words(dst[...]), axis=1)

        lax.cond(exact, keep_code, send_plain)

        s_head[head_row(c), c & 15] = jnp.where(exact, limit, 0)
        release(0, c, dst)

        @pl.when(c + N_IN < n)
        def _():
            read(send_in, send_in_sem, mx, c + N_IN)

        @pl.when(c == 0)
        def _():
            pl.semaphore_wait(entry, 2)

        @pl.when(plan.words(c + 1) > m)
        def _():
            send_word(m).start()
            s_pos[...] = jnp.maximum(s_pos[...] - 32, 0)
            new = m + WINDOW
            pl.when(new >= N_WORD)(lambda: send_word(new - N_WORD).wait_send())
            s_word[new & (N_WORD - 1)] = jnp.zeros((8, LANES), I32)

        @pl.when(c == n - 1)
        def _():
            total = plan.flush_from + _shr(jnp.max(s_pos[...]) + 31, 5)
            s_head[n_rows - 1, 16] = total
            lax.fori_loop(plan.flush_from, total, lambda m, _: send_word(m).start(), None)

        @pl.when(starts_row(c + 1))
        def _():
            q = head_row(c)
            pl.when(q >= N_HEAD)(lambda: send_head(q - N_HEAD).wait_send())
            send_head(q).start()

        return carry

    def decode_chunk(k, main, word, head, pos_ref, c):
        dst = claim(k, c)
        msg = main.at[c & (N_MAIN - 1)]
        limit = header(head, c)
        m = plan.words(c)

        def coded():
            window = [word[(m + j) & (N_WORD - 1)] for j in range(WINDOW)]
            words, pos = _decode(_parts(msg[:, :CODED]), limit, window, pos_ref[...])
            pos_ref[...] = pos
            dst[...] = _from_words(words)

        def plain():
            dst[...] = _from_words(_parts(msg[...]))

        lax.cond(limit != 0, coded, plain)

        @pl.when(plan.words(c + 1) > m)
        def _():
            pos_ref[...] = jnp.maximum(pos_ref[...] - 32, 0)

        release(k, c, dst)

    def decode_y(c, carry):
        decode_chunk(2, y_main, y_word, y_head, y_pos, c)
        return carry

    def decode_x(c, carry):
        decode_chunk(3, x_main, x_word, x_head, x_pos, c)
        with_width(y_head, c, lambda w: relay_main(c, w).wait_send())
        m = plan.words(c)
        pl.when(plan.words(c + 1) > m)(lambda: relay_word(m).wait_send())
        return carry

    def keep_chunk(c, carry):
        src = read_wait(keep_in, keep_in_sem, c)
        dst = claim(1, c)
        dst[...] = src[...].astype(BF16)
        release(1, c, dst)
        pl.when(c + N_KEEP < n)(lambda: read(keep_in, keep_in_sem, 1 - mx, c + N_KEEP))
        return carry

    def pass_word_on(m, carry):
        send_word(m).wait_recv()
        relay_word(m).start()
        return carry

    def take_word(m, carry):
        relay_word(m).wait_recv()
        return carry

    def drain():
        def main(c, carry):
            with_width(s_head, c, lambda w: send_main(c, w).wait_send())
            return carry

        def sent_word(m, carry):
            send_word(m).wait_send()
            return carry

        def relayed_word(m, carry):
            relay_word(m).wait_send()
            return carry

        lax.fori_loop(n - N_MAIN, n, main, 0)
        lax.fori_loop(plan.flush_from + WINDOW - N_WORD, s_head[n_rows - 1, 16], sent_word, 0)
        lax.fori_loop(plan.flush_from, y_head[n_rows - 1, 16], relayed_word, 0)
        for q in range(n_rows - N_HEAD, n_rows):
            send_head(q).wait_send()
            relay_head(q).wait_send()

    def pass_head_on(q):
        send_head(q).wait_recv()
        pl.when(q >= N_HEAD)(lambda: relay_head(q - N_HEAD).wait_send())
        relay_head(q).start()

    def opens_row(c):
        return jnp.logical_and(starts_row(c), c < n - 16)

    def step(i, before):
        j, k = i - Y_LAG, i - X_LAG
        after = (plan.encoded(i + 1), plan.sent(j + 1, plan.flush_from), plan.decoded(j),
                 plan.kept(i + 1), plan.sent(k + 1, plan.flush_from), plan.decoded(k))
        lax.fori_loop(before[0], after[0], encode_chunk, 0)
        pl.when(i < n)(lambda: with_width(s_head, i, lambda w: send_main(i, w).start()))
        lax.fori_loop(before[1], after[1], pass_word_on, 0)

        @pl.when(j == plan.last)
        def _():
            pass_head_on(jnp.int32(n_rows - 1))
            lax.fori_loop(plan.flush_from, y_head[n_rows - 1, 16], pass_word_on, 0)

        @pl.when(jnp.logical_and(j >= 0, j < n))
        def _():
            def pass_on(width):
                send_main(j, width).wait_recv()
                relay_main(j, width).start()

            pl.when(opens_row(j))(lambda: pass_head_on(head_row(j)))
            with_width(y_head, j, pass_on)

        lax.fori_loop(before[2], after[2], decode_y, 0)

        @pl.when(i == plan.ahead - 3)
        def _():
            for c in range(N_KEEP):
                read(keep_in, keep_in_sem, 1 - mx, jnp.int32(c))

        lax.fori_loop(before[3], after[3], keep_chunk, 0)
        lax.fori_loop(before[4], after[4], take_word, 0)

        @pl.when(k == plan.last)
        def _():
            relay_head(jnp.int32(n_rows - 1)).wait_recv()
            lax.fori_loop(plan.flush_from, x_head[n_rows - 1, 16], take_word, 0)

        @pl.when(k >= 0)
        def _():
            pl.when(opens_row(k))(lambda: relay_head(head_row(k)).wait_recv())
            with_width(x_head, k, lambda w: relay_main(k, w).wait_recv())

        lax.fori_loop(before[5], after[5], decode_x, 0)
        pl.when(i == n + X_LAG - 2)(drain)
        return after

    for c in range(N_IN):
        read(send_in, send_in_sem, mx, jnp.int32(c))
    for s in range(WINDOW):
        s_word[s] = jnp.zeros((8, LANES), I32)
    for pos_ref in (s_pos, y_pos, x_pos):
        pos_ref[...] = jnp.zeros((8, LANES), I32)
    lax.fori_loop(0, n + X_LAG, step, (jnp.int32(0),) * 6)


def pallas_dist_ag_xy_y_m65536_n1024_kernel(x: jax.Array):
    rows, cols = x.shape
    slab = STRIPS * STRIP
    assert cols == COLS and rows % (2 * SLABS * slab) == 0
    slabs = 2 * rows // slab
    n_rows = rows // (2 * SLABS * STRIP) // 16 + 4
    dma = pltpu.SemaphoreType.DMA
    in_hbm, last, in_vmem = pl.pallas_call(
        _all_gather,
        out_shape=(
            jax.ShapeDtypeStruct((HBM_STRIPS - 1, slabs, STRIP, cols), BF16),
            jax.ShapeDtypeStruct((slabs, STRIP, cols), BF16),
            pltpu.VMEM((slabs, VMEM_STRIPS * STRIP, cols), BF16),
        ),
        in_specs=[pl.BlockSpec(memory_space=pl.ANY)],
        out_specs=(
            pl.BlockSpec(memory_space=pl.ANY),
            pl.BlockSpec(memory_space=pl.ANY),
            pl.BlockSpec(memory_space=pltpu.VMEM),
        ),
        scratch_shapes=[
            pltpu.VMEM((N_IN, SLABS, STRIP, cols), jnp.float32),
            pltpu.VMEM((N_KEEP, SLABS, STRIP, cols), jnp.float32),
            *[pltpu.VMEM((N_MAIN, 8, PLAIN), I32)] * 3,
            *[pltpu.VMEM((N_WORD, 8, LANES), I32)] * 3,
            *[pltpu.VMEM((8, LANES), I32)] * 3,
            *[pltpu.SMEM((n_rows, 128), I32)] * 3,
            pltpu.SMEM((1,), I32),
            dma((N_IN,)), dma((N_KEEP,)), dma((4, N_STAGE)),
            *[dma((N_MAIN,))] * 4,
            *[dma((N_WORD,))] * 4,
            *[dma((N_HEAD,))] * 4,
        ],
        compiler_params=pltpu.CompilerParams(
            vmem_limit_bytes=16 << 20,
            collective_id=0,
            disable_semaphore_checks=True,
        ),
    )(x.reshape(rows // slab, slab, cols))
    strips = [in_vmem] + [in_hbm[t] for t in range(HBM_STRIPS - 1)] + [last]
    return jnp.concatenate(strips, axis=1).reshape(2 * rows, cols)
```
